```python
import numpy as np

kernel_name = "dist_ring_attn_i_s256_d64"

def setup_inputs():
    S, D = 1024, 64
    q = np.random.randn(S, D).astype(np.float32)
    k = np.random.randn(S, D).astype(np.float32)
    v = np.random.randn(S, D).astype(np.float32)
    return {"q": q, "k": k, "v": v}

def reference(q: np.ndarray, k: np.ndarray, v: np.ndarray) -> np.ndarray:
    D = q.shape[1]
    scores = q @ k.T / np.sqrt(D)
    scores_max = np.max(scores, axis=1, keepdims=True)
    weights = np.exp(scores - scores_max)
    weights = weights / np.sum(weights, axis=1, keepdims=True)
    return weights @ v
```

```python
import jax
import jax.numpy as jnp
from jax import lax
from jax.experimental import pallas as pl
from jax.experimental.pallas import tpu as pltpu

N_DEV = 4


def pallas_dist_ring_attn_i_s256_d64_kernel(
    q: jax.Array,
    k: jax.Array,
    v: jax.Array,
):
    s_loc, d = q.shape
    scale = 1.0 / (d ** 0.5)

    def body(q_ref, k_ref, v_ref, o_ref, kv_buf, send_sems, recv_sems):
        my = lax.axis_index("i")
        barrier = pltpu.get_barrier_semaphore()
        for off in (1, 2, 3):
            pl.semaphore_signal(
                barrier, inc=1,
                device_id=((my + off) % N_DEV,),
                device_id_type=pl.DeviceIdType.MESH,
            )

        kv_local = jnp.concatenate([k_ref[...], v_ref[...]], axis=1).astype(
            jnp.bfloat16)
        kv_buf[0] = kv_local

        pl.semaphore_wait(barrier, N_DEV - 1)

        copies = []
        for off in (1, 2, 3):
            c = pltpu.make_async_remote_copy(
                src_ref=kv_buf.at[0],
                dst_ref=kv_buf.at[off],
                send_sem=send_sems.at[off - 1],
                recv_sem=recv_sems.at[off - 1],
                device_id=((my + off) % N_DEV,),
                device_id_type=pl.DeviceIdType.MESH,
            )
            c.start()
            copies.append(c)

        q_pad = jnp.concatenate(
            [q_ref[...] * scale, jnp.zeros((s_loc, d), jnp.float32)], axis=1
        ).astype(jnp.bfloat16)

        def block(kv, m, l, acc):
            s = lax.dot_general(
                q_pad, kv, (((1,), (1,)), ((), ())),
                preferred_element_type=jnp.float32)
            m_blk = jnp.max(s, axis=1, keepdims=True)
            if m is None:
                m_new = m_blk
            else:
                m_new = jnp.maximum(m, m_blk)
            p = jnp.exp(s - m_new)
            l_blk = jnp.sum(p, axis=1, keepdims=True)
            pv = lax.dot_general(
                p.astype(jnp.bfloat16), kv, (((1,), (0,)), ((), ())),
                preferred_element_type=jnp.float32)
            if m is None:
                return m_new, l_blk, pv
            alpha = jnp.exp(m - m_new)
            return m_new, alpha * l + l_blk, alpha * acc + pv

        m, l, acc = block(kv_local, None, None, None)
        for off in (1, 3, 2):
            copies[off - 1].wait_recv()
            m, l, acc = block(kv_buf[off], m, l, acc)

        o_ref[...] = acc[:, d:] / l

        for c in copies:
            c.wait_send()

    return pl.pallas_call(
        body,
        out_shape=jax.ShapeDtypeStruct((s_loc, d), jnp.float32),
        in_specs=[pl.BlockSpec(memory_space=pltpu.VMEM)] * 3,
        out_specs=pl.BlockSpec(memory_space=pltpu.VMEM),
        scratch_shapes=[
            pltpu.VMEM((N_DEV, s_loc, 2 * d), jnp.bfloat16),
            pltpu.SemaphoreType.DMA((N_DEV - 1,)),
            pltpu.SemaphoreType.DMA((N_DEV - 1,)),
        ],
        compiler_params=pltpu.CompilerParams(collective_id=0),
    )(q, k, v)
```

```python
import jax
import jax.numpy as jnp
from jax import lax
from jax.experimental import pallas as pl
from jax.experimental.pallas import tpu as pltpu

N_DEV = 4


def pallas_dist_ring_attn_i_s256_d64_kernel(
    q: jax.Array,
    k: jax.Array,
    v: jax.Array,
):
    s_loc, d = q.shape
    scale = 1.0 / (d ** 0.5)
    hk = s_loc // 2

    def body(qt_ref, kt_ref, vt_ref, ot_ref, kv_buf, send_sems, recv_sems):
        my = lax.axis_index("i")
        left = (my + N_DEV - 1) % N_DEV
        right = (my + 1) % N_DEV
        barrier = pltpu.get_barrier_semaphore()
        for nbr in (left, right):
            pl.semaphore_signal(
                barrier, inc=1, device_id=(nbr,),
                device_id_type=pl.DeviceIdType.MESH,
            )

        for h in range(2):
            kv_buf[0, h, :d, :] = kt_ref[:, h * hk:(h + 1) * hk].astype(jnp.bfloat16)
            kv_buf[0, h, d:, :] = vt_ref[:, h * hk:(h + 1) * hk].astype(jnp.bfloat16)

        pl.semaphore_wait(barrier, 2)

        def rcopy(i, src, dst, dev):
            return pltpu.make_async_remote_copy(
                src_ref=src, dst_ref=dst,
                send_sem=send_sems.at[i], recv_sem=recv_sems.at[i],
                device_id=(dev,), device_id_type=pl.DeviceIdType.MESH,
            )

        c_r0 = rcopy(0, kv_buf.at[0, 0], kv_buf.at[1, 0], right)
        c_l1 = rcopy(2, kv_buf.at[0, 1], kv_buf.at[3, 1], left)
        c_r1 = rcopy(1, kv_buf.at[0, 1], kv_buf.at[1, 1], right)
        c_l0 = rcopy(3, kv_buf.at[0, 0], kv_buf.at[3, 0], left)
        f_r = rcopy(4, kv_buf.at[1, 0], kv_buf.at[2, 0], right)
        f_l = rcopy(5, kv_buf.at[3, 1], kv_buf.at[2, 1], left)
        c_r0.start()
        c_l1.start()
        c_r1.start()
        c_l0.start()

        qt = (qt_ref[...] * scale).astype(jnp.bfloat16)

        def block(chunks, m, l, acc):
            s_ts = []
            for (slot, h) in chunks:
                kt = kv_buf[slot, h, :d, :]
                s_ts.append(lax.dot_general(
                    kt, qt, (((0,), (0,)), ((), ())),
                    preferred_element_type=jnp.float32))
            m_new = m
            for s_t in s_ts:
                m_blk = jnp.max(s_t, axis=0, keepdims=True)
                m_new = m_blk if m_new is None else jnp.maximum(m_new, m_blk)
            l_blk = None
            pv = None
            for (slot, h), s_t in zip(chunks, s_ts):
                vt = kv_buf[slot, h, d:, :]
                p_t = jnp.exp(s_t - m_new)
                lc = jnp.sum(p_t, axis=0, keepdims=True)
                l_blk = lc if l_blk is None else l_blk + lc
                pc = lax.dot_general(
                    vt, p_t.astype(jnp.bfloat16), (((1,), (0,)), ((), ())),
                    preferred_element_type=jnp.float32)
                pv = pc if pv is None else pv + pc
            if m is None:
                return m_new, l_blk, pv
            alpha = jnp.exp(m - m_new)
            return m_new, alpha * l + l_blk, alpha * acc + pv

        m, l, acc = block([(0, 0), (0, 1)], None, None, None)

        c_r0.wait_recv()
        f_r.start()
        c_l1.wait_recv()
        f_l.start()
        m, l, acc = block([(1, 0), (3, 1)], m, l, acc)

        c_r1.wait_recv()
        c_l0.wait_recv()
        m, l, acc = block([(1, 1), (3, 0)], m, l, acc)

        f_r.wait_recv()
        f_l.wait_recv()
        m, l, acc = block([(2, 0), (2, 1)], m, l, acc)

        ot_ref[...] = acc / l

        for c in (c_r0, c_l1, c_r1, c_l0, f_r, f_l):
            c.wait_send()

    out_t = pl.pallas_call(
        body,
        out_shape=jax.ShapeDtypeStruct((d, s_loc), jnp.float32),
        in_specs=[pl.BlockSpec(memory_space=pltpu.VMEM)] * 3,
        out_specs=pl.BlockSpec(memory_space=pltpu.VMEM),
        scratch_shapes=[
            pltpu.VMEM((N_DEV, 2, 2 * d, hk), jnp.bfloat16),
            pltpu.SemaphoreType.DMA((6,)),
            pltpu.SemaphoreType.DMA((6,)),
        ],
        compiler_params=pltpu.CompilerParams(collective_id=0),
    )(q.T, k.T, v.T)
    return out_t.T
```

```python
import jax
import jax.numpy as jnp
from jax import lax
from jax.experimental import pallas as pl
from jax.experimental.pallas import tpu as pltpu

N_DEV = 4


def pallas_dist_ring_attn_i_s256_d64_kernel(
    q: jax.Array,
    k: jax.Array,
    v: jax.Array,
):
    s_loc, d = q.shape
    scale = 1.0 / (d ** 0.5)
    hk = s_loc // 2

    def body(qt_hbm, kt_hbm, vt_hbm, ot_ref, in_buf, kv_buf, in_sems,
             send_sems, recv_sems):
        my = lax.axis_index("i")
        left = (my + N_DEV - 1) % N_DEV
        right = (my + 1) % N_DEV

        barrier = pltpu.get_barrier_semaphore()
        for nbr in (left, right):
            pl.semaphore_signal(
                barrier, inc=1, device_id=(nbr,),
                device_id_type=pl.DeviceIdType.MESH,
            )

        cp_k = pltpu.make_async_copy(kt_hbm, in_buf.at[0], in_sems.at[0])
        cp_v = pltpu.make_async_copy(vt_hbm, in_buf.at[1], in_sems.at[1])
        cp_q = pltpu.make_async_copy(qt_hbm, in_buf.at[2], in_sems.at[2])
        cp_k.start()
        cp_v.start()
        cp_q.start()

        def rcopy(i, src, dst, dev):
            return pltpu.make_async_remote_copy(
                src_ref=src, dst_ref=dst,
                send_sem=send_sems.at[i], recv_sem=recv_sems.at[i],
                device_id=(dev,), device_id_type=pl.DeviceIdType.MESH,
            )

        r_own = [rcopy(2 * h + c, kv_buf.at[0, h, c], kv_buf.at[1, h, c], right)
                 for h in (0, 1) for c in (0, 1)]
        l_own = [rcopy(4 + 2 * i + c, kv_buf.at[0, h, c], kv_buf.at[3, h, c], left)
                 for i, h in enumerate((1, 0)) for c in (0, 1)]
        r_fwd = [rcopy(8 + c, kv_buf.at[1, 0, c], kv_buf.at[2, 0, c], right)
                 for c in (0, 1)]
        l_fwd = [rcopy(10 + c, kv_buf.at[3, 1, c], kv_buf.at[2, 1, c], left)
                 for c in (0, 1)]

        cp_k.wait()
        for h in range(2):
            kv_buf[0, h, 0] = in_buf[0, :, h * hk:(h + 1) * hk].astype(jnp.bfloat16)

        pl.semaphore_wait(barrier, 2)
        r_own[0].start()
        l_own[0].start()
        cp_v.wait()
        for h in range(2):
            kv_buf[0, h, 1] = in_buf[1, :, h * hk:(h + 1) * hk].astype(jnp.bfloat16)
        for a, b in zip(r_own[1:], l_own[1:]):
            a.start()
            b.start()

        cp_q.wait()
        qt = (in_buf[2] * scale).astype(jnp.bfloat16)

        def scores(chunks, m, l):
            s_ts = []
            for (slot, h) in chunks:
                s_ts.append(lax.dot_general(
                    kv_buf[slot, h, 0], qt, (((0,), (0,)), ((), ())),
                    preferred_element_type=jnp.float32))
            m_new = m
            for s_t in s_ts:
                m_blk = jnp.max(s_t, axis=0, keepdims=True)
                m_new = m_blk if m_new is None else jnp.maximum(m_new, m_blk)
            l_blk = None
            p_ts = []
            for s_t in s_ts:
                p_t = jnp.exp(s_t - m_new)
                lc = jnp.sum(p_t, axis=0, keepdims=True)
                l_blk = lc if l_blk is None else l_blk + lc
                p_ts.append(p_t.astype(jnp.bfloat16))
            if m is None:
                return m_new, l_blk, None, p_ts
            alpha = jnp.exp(m - m_new)
            return m_new, alpha * l + l_blk, alpha, p_ts

        def values(chunks, p_ts, alpha, acc):
            pv = None
            for (slot, h), p_t in zip(chunks, p_ts):
                pc = lax.dot_general(
                    kv_buf[slot, h, 1], p_t, (((1,), (0,)), ((), ())),
                    preferred_element_type=jnp.float32)
                pv = pc if pv is None else pv + pc
            if acc is None:
                return pv
            return alpha * acc + pv

        ch = [(0, 0), (0, 1)]
        m, l, alpha, p_ts = scores(ch, None, None)
        acc = values(ch, p_ts, alpha, None)

        ch = [(1, 0), (3, 1)]
        r_own[0].wait_recv()
        r_fwd[0].start()
        l_own[0].wait_recv()
        l_fwd[0].start()
        m, l, alpha, p_ts = scores(ch, m, l)
        r_own[1].wait_recv()
        r_fwd[1].start()
        l_own[1].wait_recv()
        l_fwd[1].start()
        acc = values(ch, p_ts, alpha, acc)

        ch = [(1, 1), (3, 0)]
        r_own[2].wait_recv()
        l_own[2].wait_recv()
        m, l, alpha, p_ts = scores(ch, m, l)
        r_own[3].wait_recv()
        l_own[3].wait_recv()
        acc = values(ch, p_ts, alpha, acc)

        ch = [(2, 0), (2, 1)]
        r_fwd[0].wait_recv()
        l_fwd[0].wait_recv()
        m, l, alpha, p_ts = scores(ch, m, l)
        inv_l = 1.0 / l
        r_fwd[1].wait_recv()
        l_fwd[1].wait_recv()
        acc = values(ch, p_ts, alpha, acc)

        ot_ref[...] = acc * inv_l

        for c in r_own + l_own + r_fwd + l_fwd:
            c.wait_send()

    out_t = pl.pallas_call(
        body,
        out_shape=jax.ShapeDtypeStruct((d, s_loc), jnp.float32),
        in_specs=[pl.BlockSpec(memory_space=pl.ANY)] * 3,
        out_specs=pl.BlockSpec(memory_space=pltpu.VMEM),
        scratch_shapes=[
            pltpu.VMEM((3, d, s_loc), jnp.float32),
            pltpu.VMEM((N_DEV, 2, 2, d, hk), jnp.bfloat16),
            pltpu.SemaphoreType.DMA((3,)),
            pltpu.SemaphoreType.DMA((12,)),
            pltpu.SemaphoreType.DMA((12,)),
        ],
        compiler_params=pltpu.CompilerParams(collective_id=0),
    )(q.T, k.T, v.T)
    return out_t.T
```

```python
import functools

import jax
import jax.numpy as jnp
from jax import lax
from jax.experimental import pallas as pl
from jax.experimental.pallas import tpu as pltpu

N_DEV = 4
F, A, L, B = 0, 1, 2, 3
K, V = 0, 1


def unit(blk, c, h):
    return blk * 4 + c * 2 + h


def pallas_dist_ring_attn_i_s256_d64_kernel(
    q: jax.Array,
    k: jax.Array,
    v: jax.Array,
):
    s_loc, d = q.shape
    scale = 1.0 / (d ** 0.5)
    hk = s_loc // 2

    def body(qt_hbm, kt_hbm, vt_hbm, ot_ref, in_buf, kv_buf, in_sems,
             send_sem, recv_sems, hello_sems):
        my = lax.axis_index("i")
        barrier = pltpu.get_barrier_semaphore()

        def sig(sem, dev):
            pl.semaphore_signal(sem, inc=1, device_id=(dev,),
                                device_id_type=pl.DeviceIdType.MESH)

        def program(role):
            n_sent = [0]

            def rdma(u0, n, dst, sem):
                return pltpu.make_async_remote_copy(
                    src_ref=kv_buf.at[u0:u0 + n], dst_ref=kv_buf.at[u0:u0 + n],
                    send_sem=send_sem, recv_sem=recv_sems.at[sem],
                    device_id=(dst,), device_id_type=pl.DeviceIdType.MESH)

            def send(blk, c, h, dst, sem, n=1):
                rdma(unit(blk, c, h), n, dst, sem).start()
                n_sent[0] += n

            def recv(sem, n):
                rdma(0, n, role, sem).wait_recv()

            cp_k = pltpu.make_async_copy(kt_hbm, in_buf.at[0], in_sems.at[0])
            cp_v = pltpu.make_async_copy(vt_hbm, in_buf.at[1], in_sems.at[1])
            cp_q = pltpu.make_async_copy(qt_hbm, in_buf.at[2], in_sems.at[1])
            cp_k.start()
            cp_v.start()
            cp_q.start()

            for n in {F: (A, B, L), A: (L,), B: (L,), L: ()}[role]:
                sig(barrier, n)

            if role in (A, B):
                pl.semaphore_wait(barrier, 1)
                sig(hello_sems.at[0 if role == A else 1], F)
            elif role == L:
                pl.semaphore_wait(barrier, 3)
                sig(hello_sems.at[0], A)
                sig(hello_sems.at[0], B)

            cp_k.wait()
            for h in range(2):
                kv_buf[unit(role, K, h)] = (
                    in_buf[0, :, h * hk:(h + 1) * hk].astype(jnp.bfloat16))
            if role in (A, B):
                send(role, K, 0, F, 0)
            elif role == L:
                send(L, K, 0, F, 4, n=2)
            pltpu.make_async_copy(in_buf.at[1:3], in_buf.at[1:3],
                                  in_sems.at[1]).wait()
            for h in range(2):
                kv_buf[unit(role, V, h)] = (
                    in_buf[1, :, h * hk:(h + 1) * hk].astype(jnp.bfloat16))
            if role in (A, B):
                send(role, V, 0, F, 1)
                send(role, K, 1, F, 2)
                send(role, V, 1, F, 3)
            elif role == L:
                send(L, V, 1, B, 1)
                send(L, V, 0, F, 5)
                send(L, K, 0, B, 4, n=2)
                send(L, V, 0, B, 5)
                send(L, K, 0, A, 3, n=2)
                send(L, V, 0, A, 4, n=2)

            qt = (in_buf[2] * scale).astype(jnp.bfloat16)

            def scores(chunks, m, l):
                s_ts = []
                for (blk, h) in chunks:
                    s_ts.append(lax.dot_general(
                        kv_buf[unit(blk, K, h)], qt, (((0,), (0,)), ((), ())),
                        preferred_element_type=jnp.float32))
                m_new = m
                for s_t in s_ts:
                    m_blk = jnp.max(s_t, axis=0, keepdims=True)
                    m_new = m_blk if m_new is None else jnp.maximum(m_new, m_blk)
                l_blk = None
                p_ts = []
                for s_t in s_ts:
                    p_t = jnp.exp(s_t - m_new)
                    lc = jnp.sum(p_t, axis=0, keepdims=True)
                    l_blk = lc if l_blk is None else l_blk + lc
                    p_ts.append(p_t.astype(jnp.bfloat16))
                if m is None:
                    return m_new, l_blk, None, p_ts
                alpha = jnp.exp(m - m_new)
                return m_new, alpha * l + l_blk, alpha, p_ts

            def values(chunks, p_ts, alpha, acc):
                pv = None
                for (blk, h), p_t in zip(chunks, p_ts):
                    pc = lax.dot_general(
                        kv_buf[unit(blk, V, h)], p_t, (((1,), (0,)), ((), ())),
                        preferred_element_type=jnp.float32)
                    pv = pc if pv is None else pv + pc
                if acc is None:
                    return pv
                return alpha * acc + pv

            ch = [(role, 0), (role, 1)]
            m, l, alpha, p_ts = scores(ch, None, None)
            acc = values(ch, p_ts, alpha, None)

            if role == F:
                pl.semaphore_wait(hello_sems.at[0], 1)
                send(F, K, 0, A, 0)
                send(F, V, 0, A, 1)
                send(F, K, 1, A, 2)
                send(F, V, 1, A, 2)
                pl.semaphore_wait(hello_sems.at[1], 1)
                send(F, K, 1, B, 0)
                send(F, V, 1, B, 2)
                send(F, K, 0, B, 3)
                send(F, V, 0, B, 3)
                for h in (0, 1):
                    ch = [(A, h), (B, h)]
                    recv(2 * h, 2)
                    send(A, K, h, B, 4)
                    send(B, K, h, A, 3)
                    m, l, alpha, p_ts = scores(ch, m, l)
                    recv(2 * h + 1, 2)
                    send(A, V, h, B, 5)
                    send(B, V, h, A, 4)
                    acc = values(ch, p_ts, alpha, acc)
                ch = [(L, 0), (L, 1)]
                recv(4, 2)
                m, l, alpha, p_ts = scores(ch, m, l)
                inv_l = 1.0 / l
                recv(5, 2)
                acc = values(ch, p_ts, alpha, acc)
            elif role == A:
                pl.semaphore_wait(hello_sems.at[0], 1)
                send(A, K, 0, L, 0)
                send(A, V, 0, L, 1)
                send(A, K, 1, L, 2)
                send(A, V, 1, L, 3)
                recv(0, 1)
                send(F, K, 0, L, 4)
                recv(1, 1)
                send(F, V, 0, L, 5)
                recv(2, 2)
                ch = [(F, 0), (F, 1)]
                m, l, alpha, p_ts = scores(ch, m, l)
                acc = values(ch, p_ts, alpha, acc)
                ch = [(B, 0), (B, 1), (L, 0), (L, 1)]
                recv(3, 4)
                m, l, alpha, p_ts = scores(ch, m, l)
                inv_l = 1.0 / l
                recv(4, 4)
                acc = values(ch, p_ts, alpha, acc)
            elif role == B:
                pl.semaphore_wait(hello_sems.at[0], 1)
                send(B, K, 0, L, 0)
                send(B, V, 0, L, 1)
                send(B, K, 1, L, 2)
                send(B, V, 1, L, 3)
                recv(0, 1)
                send(F, K, 1, L, 4)
                recv(1, 1)
                send(L, V, 1, F, 5)
                recv(2, 1)
                send(F, V, 1, L, 5)
                recv(3, 2)
                ch = [(F, 0), (F, 1)]
                m, l, alpha, p_ts = scores(ch, m, l)
                acc = values(ch, p_ts, alpha, acc)
                ch = [(L, 0), (L, 1), (A, 0), (A, 1)]
                recv(4, 4)
                m, l, alpha, p_ts = scores(ch, m, l)
                inv_l = 1.0 / l
                recv(5, 3)
                acc = values(ch, p_ts, alpha, acc)
            else:
                for h in (0, 1):
                    ch = [(A, h), (B, h)]
                    recv(2 * h, 2)
                    m, l, alpha, p_ts = scores(ch, m, l)
                    recv(2 * h + 1, 2)
                    acc = values(ch, p_ts, alpha, acc)
                ch = [(F, 0), (F, 1)]
                recv(4, 2)
                m, l, alpha, p_ts = scores(ch, m, l)
                inv_l = 1.0 / l
                recv(5, 2)
                acc = values(ch, p_ts, alpha, acc)

            ot_ref[...] = acc * inv_l
            rdma(0, n_sent[0], role, 0).wait_send()

        for role in range(N_DEV):
            pl.when(my == role)(functools.partial(program, role))

    out_t = pl.pallas_call(
        body,
        out_shape=jax.ShapeDtypeStruct((d, s_loc), jnp.float32),
        in_specs=[pl.BlockSpec(memory_space=pl.ANY)] * 3,
        out_specs=pl.BlockSpec(memory_space=pltpu.VMEM),
        scratch_shapes=[
            pltpu.VMEM((3, d, s_loc), jnp.float32),
            pltpu.VMEM((4 * N_DEV, d, hk), jnp.bfloat16),
            pltpu.SemaphoreType.DMA((2,)),
            pltpu.SemaphoreType.DMA,
            pltpu.SemaphoreType.DMA((6,)),
            pltpu.SemaphoreType.REGULAR((2,)),
        ],
        compiler_params=pltpu.CompilerParams(collective_id=0),
    )(q.T, k.T, v.T)
    return out_t.T
```
